```python
import numpy as np

kernel_name = "dist_ring_attn_i_s256_d64"

def setup_inputs():
    S, D = 1024, 64
    q = np.random.randn(S, D).astype(np.float32)
    k = np.random.randn(S, D).astype(np.float32)
    v = np.random.randn(S, D).astype(np.float32)
    return {"q": q, "k": k, "v": v}

def reference(q: np.ndarray, k: np.ndarray, v: np.ndarray) -> np.ndarray:
    D = q.shape[1]
    scores = q @ k.T / np.sqrt(D)
    scores_max = np.max(scores, axis=1, keepdims=True)
    weights = np.exp(scores - scores_max)
    weights = weights / np.sum(weights, axis=1, keepdims=True)
    return weights @ v
```

```python
import functools

import jax
import jax.numpy as jnp
from jax import lax
from jax.experimental import pallas as pl
from jax.experimental.pallas import tpu as pltpu

_N_DEV = 4
_MESH = pl.DeviceIdType.MESH
_LOG2E = 1.4426950408889634
_BF16, _F32 = jnp.bfloat16, jnp.float32

_K = ("K", 0, 128)
_K_LO, _K_HI = ("K", 0, 64), ("K", 64, 64)
_VA, _VB = ("V", 0, 32), ("V", 32, 32)
_V0, _V1, _V2, _V3 = (("V", r, 16) for r in (0, 16, 32, 48))


def _send(dst, *pieces):
    return [("send", dst, p) for p in pieces]


def _recv(src, *pieces):
    return [("recv", src, p) for p in pieces]


def _relay(src, piece, dst):
    return [("recv", src, piece), ("relay", src, piece, dst)]


def _own(me):
    return [("prep_q",), ("scores", (me,)), ("pv", me)]


def _block(src, v_pieces=(_VA, _VB)):
    return _recv(src, _K) + [("scores", (src,))] + _recv(src, *v_pieces) + [("pv", src)]


def _last_block(src):
    return (
        _recv(src, _K)
        + [("scores", (src,)), ("inv",), ("drain",)]
        + _recv(src, _VA, _VB)
        + [("pv_out", src)]
    )


def _last_two_blocks(a, b):
    return (
        _recv(a, _K)
        + _recv(b, _K)
        + [("scores", (a, b)), ("inv",)]
        + _recv(a, _VA, _VB)
        + [("pv", a), ("drain",)]
        + _recv(b, _VA, _VB)
        + [("pv_out", b)]
    )


def _odd_chip_prologue():
    return (
        [("enter", (0, 2)), ("prep_v", _VA), ("wait_enter", 1)]
        + _send(0, _VA)
        + [("prep_k",)]
        + _send(0, _K)
        + [("prep_v", _VB)]
        + _send(0, _VB)
    )


_PLANS = (
    [("enter", (1, 3, 2)), ("prep_v", _VA), ("prep_k",), ("prep_v", _VB)]
    + _own(0)
    + [("wait_enter", 2)]
    + _send(1, _VA) + _send(3, _VA) + _send(1, _K) + _send(3, _K) + _send(1, _VB) + _send(3, _VB)
    + [("wait_go",)]
    + _send(2, _VA, _K, _VB)
    + _relay(3, _VA, 1) + _relay(3, _K, 1) + _recv(1, _K)
    + [("scores", (1, 3))]
    + _relay(3, _VB, 1) + _recv(1, _VA, _VB)
    + [("pv", 1), ("pv", 3), ("drain", 6)]
    + _recv(2, _K_LO) + [("scores_lo", 2)]
    + _recv(2, _K_HI) + [("scores", (2,)), ("drain",)]
    + _recv(2, _V0, _V1, _V2, _V3)
    + [("inv",), ("pv_out", 2)],
    _odd_chip_prologue()
    + _own(1)
    + [("wait_go",)]
    + _send(3, _VA, _K, _VB) + _send(2, _VA, _K, _VB)
    + _block(0)
    + _last_two_blocks(2, 3),
    [("wait_enter", 3), ("go", (1, 3, 0)), ("prep_v", _VA)]
    + _send(3, _V0, _V1)
    + [("prep_k_start",), ("prep_v", _VB)]
    + _send(3, _V2)
    + [("prep_k_finish",)]
    + _send(0, _K_LO, _K_HI) + _send(3, _K) + _send(0, _V3) + _send(3, _V3)
    + _send(1, _K, _VA, _VB)
    + _own(2)
    + _block(3)
    + _last_two_blocks(0, 1),
    _odd_chip_prologue()
    + _own(3)
    + [("wait_go",)]
    + _send(2, _VA, _K, _VB)
    + _relay(2, _V0, 0) + _relay(2, _V1, 0) + _relay(2, _V2, 0)
    + _block(0)
    + _block(2, (_V3,))
    + _last_block(1),
)

_LOADS = (_VA, "k", _VB, "q")


def _recv_slots():
    slots = tuple({} for _ in range(_N_DEV))
    for me, plan in enumerate(_PLANS):
        for step in plan:
            if step[0] == "send":
                dst, key = step[1], (me, step[2])
            elif step[0] == "relay":
                dst, key = step[3], (step[1], step[2])
            else:
                continue
            assert key not in slots[dst]
            slots[dst][key] = len(slots[dst])
    for me, plan in enumerate(_PLANS):
        waited = [(s[1], s[2]) for s in plan if s[0] == "recv"]
        assert sorted(waited) == sorted(slots[me])
    return slots


_RECV_SLOT = _recv_slots()
_N_RECV = max(len(s) for s in _RECV_SLOT)
_N_SEND = max(sum(s[0] in ("send", "relay") for s in plan) for plan in _PLANS)


def _attention_kernel(
    q_hbm, k_hbm, v_hbm,
    o_ref,
    qf, kf, vf,
    kp,
    vt,
    load_sem, send_sem, recv_sem, go_sem,
):
    d, s = qf.shape
    half = s // 2
    entry_sem = pltpu.get_barrier_semaphore()

    def load(i):
        what = _LOADS[i]
        if what == "k":
            return pltpu.make_async_copy(k_hbm, kf, load_sem.at[i])
        if what == "q":
            return pltpu.make_async_copy(q_hbm, qf, load_sem.at[i])
        rows = pl.ds(what[1], what[2])
        return pltpu.make_async_copy(v_hbm.at[rows], vf.at[rows], load_sem.at[i])

    for i in range(len(_LOADS)):
        load(i).start()

    def piece_ref(src, piece):
        buf = kp if piece[0] == "K" else vt
        return buf.at[src, pl.ds(piece[1], piece[2])]

    def run(me):
        sent = []
        st = {}
        drained = 0

        def remote(src, piece, dst):
            ref = piece_ref(src, piece)
            return pltpu.make_async_remote_copy(
                ref, ref, send_sem.at[len(sent)], recv_sem.at[_RECV_SLOT[dst][src, piece]],
                device_id=(dst,), device_id_type=_MESH,
            )

        def pv_rows(src):
            p, v = st.pop(("p", src)), vt[src]
            return jnp.dot(v[:, :half], p[:, :s], preferred_element_type=_F32) + jnp.dot(
                v[:, half:], p[:, s:], preferred_element_type=_F32
            )

        def qk(rows):
            return jnp.dot(rows, st["q"], preferred_element_type=_F32)

        for step in _PLANS[me]:
            op = step[0]
            if op == "enter":
                for dst in step[1]:
                    pl.semaphore_signal(entry_sem, 1, device_id=(dst,), device_id_type=_MESH)
            elif op == "wait_enter":
                pl.semaphore_wait(entry_sem, step[1])
            elif op == "go":
                for dst in step[1]:
                    pl.semaphore_signal(go_sem, 1, device_id=(dst,), device_id_type=_MESH)
            elif op == "wait_go":
                pl.semaphore_wait(go_sem, 1)
            elif op == "prep_v":
                _, r0, n = step[1]
                load(_LOADS.index(step[1])).wait()
                vt[me, r0:r0 + n, :] = vf[r0:r0 + n, :].astype(_BF16)
            elif op in ("prep_k", "prep_k_start"):
                load(_LOADS.index("k")).wait()
                k = kf[...]
                st["kp"] = jnp.concatenate([k[:, :half], k[:, half:]], axis=0).T
                if op == "prep_k":
                    kp[me] = st.pop("kp").astype(_BF16)
            elif op == "prep_k_finish":
                kp[me] = st.pop("kp").astype(_BF16)
            elif op == "prep_q":
                load(_LOADS.index("q")).wait()
                q = (qf[...] * (_LOG2E / d**0.5)).astype(_BF16)
                z = jnp.zeros_like(q)
                st["q"] = jnp.concatenate(
                    [jnp.concatenate([q, z], axis=1), jnp.concatenate([z, q], axis=1)], axis=0
                )
            elif op == "send":
                sent.append(remote(me, step[2], step[1]))
                sent[-1].start()
            elif op == "relay":
                sent.append(remote(step[1], step[2], step[3]))
                sent[-1].start()
            elif op == "recv":
                ref = piece_ref(step[1], step[2])
                pltpu.make_async_remote_copy(
                    ref, ref, send_sem.at[0], recv_sem.at[_RECV_SLOT[me][step[1], step[2]]],
                    device_id=(step[1],), device_id_type=_MESH,
                ).wait_recv()
            elif op == "scores_lo":
                st["lo", step[1]] = qk(kp[step[1], 0:d, :])
            elif op == "scores":
                blocks = []
                for src in step[1]:
                    if ("lo", src) in st:
                        hi = qk(kp[src, d:2 * d, :])
                        blocks.append(jnp.concatenate([st.pop(("lo", src)), hi], axis=0))
                    else:
                        blocks.append(qk(kp[src]))
                m = functools.reduce(
                    jnp.maximum, [jnp.max(b, axis=0, keepdims=True) for b in blocks]
                )
                m = jnp.maximum(m[:, :s], m[:, s:])
                if "m" in st:
                    m = jnp.maximum(st["m"], m)
                probs = [jnp.exp2(b - jnp.concatenate([m, m], axis=1)) for b in blocks]
                l = functools.reduce(jnp.add, [jnp.sum(p, axis=0, keepdims=True) for p in probs])
                l = l[:, :s] + l[:, s:]
                if "m" in st:
                    alpha = jnp.exp2(st["m"] - m)
                    l = st["l"] * alpha + l
                    st["acc"] = st["acc"] * alpha
                st["m"], st["l"] = m, l
                for src, p in zip(step[1], probs):
                    st["p", src] = p.astype(_BF16)
            elif op == "pv":
                pv = pv_rows(step[1])
                st["acc"] = st["acc"] + pv if "acc" in st else pv
            elif op == "inv":
                st["inv"] = 1.0 / st["l"]
            elif op == "pv_out":
                o_ref[...] = (st["acc"] + pv_rows(step[1])) * st["inv"]
            elif op == "drain":
                upto = step[1] if len(step) > 1 else len(sent)
                for copy in sent[drained:upto]:
                    copy.wait_send()
                drained = upto
            else:
                raise ValueError(op)
        assert drained == len(sent)

    pos = lax.axis_index("i")
    for me in (2, 1, 3, 0):
        pl.when(pos == me)(functools.partial(run, me))


def pallas_dist_ring_attn_i_s256_d64_kernel(q: jax.Array, k: jax.Array, v: jax.Array):
    s, d = q.shape
    assert (s, d) == (256, 64) and k.shape == v.shape == q.shape
    in_hbm = pl.BlockSpec(memory_space=pl.ANY)
    o_t = pl.pallas_call(
        _attention_kernel,
        out_shape=jax.ShapeDtypeStruct((d, s), _F32),
        in_specs=[in_hbm, in_hbm, in_hbm],
        out_specs=pl.BlockSpec(memory_space=pltpu.VMEM),
        scratch_shapes=[
            pltpu.VMEM((d, s), _F32),
            pltpu.VMEM((d, s), _F32),
            pltpu.VMEM((d, s), _F32),
            pltpu.VMEM((_N_DEV, 2 * d, s // 2), _BF16),
            pltpu.VMEM((_N_DEV, d, s), _BF16),
            pltpu.SemaphoreType.DMA((len(_LOADS),)),
            pltpu.SemaphoreType.DMA((_N_SEND,)),
            pltpu.SemaphoreType.DMA((_N_RECV,)),
            pltpu.SemaphoreType.REGULAR,
        ],
        compiler_params=pltpu.CompilerParams(collective_id=0, disable_semaphore_checks=True),
    )(q.astype(_F32).T, k.astype(_F32).T, v.astype(_F32).T)
    return o_t.T
```
